```python
import numpy as np

kernel_name = "dist_rmsnorm_colshard_i_m768_n512"

def setup_inputs():
    x = np.random.randn(768, 2048).astype(np.float32)
    gamma = np.random.randn(2048).astype(np.float32)
    return {"x": x, "gamma": gamma}

def reference(x: np.ndarray, gamma: np.ndarray) -> np.ndarray:
    eps = 1e-5
    rms = np.sqrt(np.mean(x * x, axis=1, keepdims=True) + eps)
    return gamma * x / rms
```

```python
import jax
import jax.numpy as jnp
from jax import lax
from jax.experimental import pallas as pl
from jax.experimental.pallas import tpu as pltpu

N_DEV = 4
EPS = 1e-5
CHUNKS = (512, 192, 64)
ORDER = (2, 1, 3)


def pallas_dist_rmsnorm_colshard_i_m768_n512_kernel(
    x: jax.Array,
    gamma: jax.Array,
):
    m, n = x.shape
    chunks = CHUNKS
    assert sum(chunks) == m
    nch = len(chunks)
    offs = [sum(chunks[:i]) for i in range(nch)]
    n_glob = n * N_DEV
    g2 = gamma.reshape(1, n)

    def body(x_hbm, g_hbm, o_ref, xbuf, gbuf, comm, in_sems, g_sem, send_sem, recv_sems):
        me = lax.axis_index("i")
        ins = [
            pltpu.make_async_copy(
                x_hbm.at[pl.ds(offs[c], chunks[c])],
                xbuf.at[pl.ds(offs[c], chunks[c])],
                in_sems.at[c],
            )
            for c in range(nch)
        ]
        for cp in ins:
            cp.start()
        gcp = pltpu.make_async_copy(g_hbm, gbuf, g_sem)
        gcp.start()
        barrier = pltpu.get_barrier_semaphore()
        for d in ORDER:
            pl.semaphore_signal(
                barrier, inc=1, device_id=((me + d) % N_DEV,),
                device_id_type=pl.DeviceIdType.MESH,
            )

        lane = lax.broadcasted_iota(jnp.int32, (8, 128), 1)
        for c in range(nch):
            rows = chunks[c]
            ins[c].wait()
            xv = xbuf[pl.ds(offs[c], rows), :]
            xx = xv * xv
            p = xx[:, 0:128]
            for k in range(1, n // 128):
                p = p + xx[:, 128 * k:128 * (k + 1)]
            s = jnp.sum(p, axis=1, keepdims=True)
            acc = jnp.zeros((8, 128), jnp.float32)
            for j in range(rows // 8):
                acc = jnp.where(lane == j, s[8 * j:8 * j + 8, :], acc)
            comm[c, 0] = acc
            if c == 0:
                pl.semaphore_wait(barrier, N_DEV - 1)
            for d in ORDER:
                pltpu.make_async_remote_copy(
                    src_ref=comm.at[c, 0], dst_ref=comm.at[c, d],
                    send_sem=send_sem, recv_sem=recv_sems.at[c],
                    device_id=((me + d) % N_DEV,),
                    device_id_type=pl.DeviceIdType.MESH,
                ).start()
        gcp.wait()
        xbuf[...] = xbuf[...] * gbuf[...]
        for c in range(nch):
            rows = chunks[c]
            if c == nch - 1:
                sent = comm.at[:, pl.ds(1, N_DEV - 1)]
                pltpu.make_async_copy(sent, sent, send_sem).wait()
            got = comm.at[c, pl.ds(1, N_DEV - 1)]
            pltpu.make_async_copy(got, got, recv_sems.at[c]).wait()
            tot = comm[c, 0] + comm[c, 1] + comm[c, 2] + comm[c, 3]
            r = lax.rsqrt(tot * (1.0 / n_glob) + EPS)
            for j in range(rows // 8):
                sl = pl.ds(offs[c] + 8 * j, 8)
                o_ref[sl, :] = xbuf[sl, :] * r[:, j:j + 1]

    return pl.pallas_call(
        body,
        out_shape=jax.ShapeDtypeStruct((m, n), x.dtype),
        in_specs=[
            pl.BlockSpec(memory_space=pl.ANY),
            pl.BlockSpec(memory_space=pl.ANY),
        ],
        out_specs=pl.BlockSpec(memory_space=pltpu.VMEM),
        scratch_shapes=[
            pltpu.VMEM((m, n), jnp.float32),
            pltpu.VMEM((1, n), jnp.float32),
            pltpu.VMEM((nch, N_DEV, 8, 128), jnp.float32),
            pltpu.SemaphoreType.DMA((nch,)),
            pltpu.SemaphoreType.DMA,
            pltpu.SemaphoreType.DMA,
            pltpu.SemaphoreType.DMA((nch,)),
        ],
        compiler_params=pltpu.CompilerParams(
            collective_id=0,
            disable_semaphore_checks=True,
            disable_bounds_checks=True,
        ),
    )(x, g2)
```

```python
import jax
import jax.numpy as jnp
from jax import lax
from jax.experimental import pallas as pl
from jax.experimental.pallas import tpu as pltpu

N_DEV = 4
EPS = 1e-5
LANES = 128
SUBLANES = 8

CHUNKS = (256, 128, 128, 128, 64, 64)
N_FAST = 4
PEERS = (2, 1, 3)
SLOT = {1: 1, 3: 2, 2: 3}


def pallas_dist_rmsnorm_colshard_i_m768_n512_kernel(
    x: jax.Array,
    gamma: jax.Array,
):
    m, n = x.shape
    chunks = CHUNKS
    assert sum(chunks) == m and n % LANES == 0
    nch = len(chunks)
    offs = [sum(chunks[:c]) for c in range(nch)]
    mrows = [-(-r // LANES) for r in chunks]
    moffs = [sum(mrows[:c]) for c in range(nch)]
    mtot = sum(mrows)
    fast = [c >= nch - N_FAST for c in range(nch)]
    inv_n = 1.0 / (n * N_DEV)
    groups_per_row = LANES // SUBLANES

    def groups(c):
        for g in range(chunks[c] // SUBLANES):
            yield (
                moffs[c] + g // groups_per_row,
                SUBLANES * (g % groups_per_row),
                offs[c] + SUBLANES * g,
            )

    def body(x_hbm, g_hbm, o_ref, xbuf, gbuf, comm, sbuf, part,
             in_sems, g_sem, send_sem, recv_sems, fast_sems):
        me = lax.axis_index("i")

        loads = [
            pltpu.make_async_copy(
                x_hbm.at[pl.ds(offs[c], chunks[c])],
                xbuf.at[pl.ds(offs[c], chunks[c])],
                in_sems.at[c],
            )
            for c in range(nch)
        ]
        for cp in loads:
            cp.start()
        g_load = pltpu.make_async_copy(g_hbm, gbuf, g_sem)
        g_load.start()

        barrier = pltpu.get_barrier_semaphore()
        for d in PEERS:
            pl.semaphore_signal(
                barrier, inc=1, device_id=((me + d) % N_DEV,),
                device_id_type=pl.DeviceIdType.MESH,
            )

        lane = lax.broadcasted_iota(jnp.int32, (SUBLANES, LANES), 1)
        sub = lax.broadcasted_iota(jnp.int32, (SUBLANES, LANES), 0)
        diag = lane - sub

        def to_column(row, b):
            wide = jnp.broadcast_to(row, (SUBLANES, LANES))
            return jnp.sum(jnp.where(diag == b, wide, 0.0), axis=1, keepdims=True)

        fast_copies = {}
        for c in range(nch):
            loads[c].wait()
            xv = xbuf[pl.ds(offs[c], chunks[c]), :]
            xx = xv * xv
            cols = [xx[:, LANES * k:LANES * (k + 1)] for k in range(n // LANES)]
            while len(cols) > 1:
                nxt = [cols[i] + cols[i + 1] for i in range(0, len(cols) - 1, 2)]
                if len(cols) % 2:
                    nxt.append(cols[-1])
                cols = nxt
            ssq = jnp.sum(cols[0], axis=1, keepdims=True)
            acc = {q: jnp.zeros((SUBLANES, LANES), jnp.float32)
                   for q in range(moffs[c], moffs[c] + mrows[c])}
            for q, b, r0 in groups(c):
                r = r0 - offs[c]
                acc[q] = jnp.where(diag == b, ssq[r:r + SUBLANES, :], acc[q])
            for q, a in acc.items():
                comm[0, q] = jnp.sum(a, axis=0, keepdims=True)

            if c == 0:
                pl.semaphore_wait(barrier, N_DEV - 1)

            msg = pl.ds(moffs[c], mrows[c])
            for d in PEERS:
                to_smem = fast[c] and d == 2
                cp = pltpu.make_async_remote_copy(
                    src_ref=comm.at[0, msg],
                    dst_ref=sbuf.at[msg] if to_smem else comm.at[SLOT[d], msg],
                    send_sem=send_sem,
                    recv_sem=fast_sems.at[c] if to_smem else recv_sems.at[c],
                    device_id=((me + d) % N_DEV,),
                    device_id_type=pl.DeviceIdType.MESH,
                )
                cp.start()
                if to_smem:
                    fast_copies[c] = cp

        g_load.wait()
        xbuf[...] = xbuf[...] * gbuf[...]

        for c in range(nch):
            if not fast[c]:
                continue
            got = comm.at[pl.ds(1, 2), pl.ds(moffs[c], mrows[c])]
            pltpu.make_async_copy(got, got, recv_sems.at[c]).wait()
            near = {q: (comm[0, q] + comm[1, q] + comm[2, q]) * inv_n + EPS
                    for q in range(moffs[c], moffs[c] + mrows[c])}
            for q, b, r0 in groups(c):
                part[pl.ds(r0, SUBLANES), :] = jnp.broadcast_to(
                    to_column(near[q], b), (SUBLANES, LANES))

        for c in range(nch):
            if c == nch - 1:
                sent = comm.at[pl.ds(1, N_DEV - 1)]
                pltpu.make_async_copy(sent, sent, send_sem).wait()
            if fast[c]:
                fast_copies[c].wait_recv()
                for q, b, r0 in groups(c):
                    far = jnp.full((SUBLANES, LANES), sbuf[q, 0, b], jnp.float32)
                    for s in range(1, SUBLANES):
                        far = jnp.where(sub == s, sbuf[q, 0, b + s], far)
                    rows = pl.ds(r0, SUBLANES)
                    scale = lax.rsqrt(far * inv_n + part[rows, :])
                    for k in range(n // LANES):
                        cs = pl.ds(LANES * k, LANES)
                        o_ref[rows, cs] = xbuf[rows, cs] * scale
            else:
                got = comm.at[pl.ds(1, N_DEV - 1), pl.ds(moffs[c], mrows[c])]
                pltpu.make_async_copy(got, got, recv_sems.at[c]).wait()
                scale = {}
                for q in range(moffs[c], moffs[c] + mrows[c]):
                    tot = (comm[0, q] + comm[1, q]) + (comm[2, q] + comm[3, q])
                    scale[q] = lax.rsqrt(tot * inv_n + EPS)
                for q, b, r0 in groups(c):
                    rows = pl.ds(r0, SUBLANES)
                    o_ref[rows, :] = xbuf[rows, :] * to_column(scale[q], b)

    return pl.pallas_call(
        body,
        out_shape=jax.ShapeDtypeStruct((m, n), x.dtype),
        in_specs=[
            pl.BlockSpec(memory_space=pl.ANY),
            pl.BlockSpec(memory_space=pl.ANY),
        ],
        out_specs=pl.BlockSpec(memory_space=pltpu.VMEM),
        scratch_shapes=[
            pltpu.VMEM((m, n), jnp.float32),
            pltpu.VMEM((1, n), jnp.float32),
            pltpu.VMEM((N_DEV, mtot, 1, LANES), jnp.float32),
            pltpu.SMEM((mtot, 1, LANES), jnp.float32),
            pltpu.VMEM((m, LANES), jnp.float32),
            pltpu.SemaphoreType.DMA((nch,)),
            pltpu.SemaphoreType.DMA,
            pltpu.SemaphoreType.DMA,
            pltpu.SemaphoreType.DMA((nch,)),
            pltpu.SemaphoreType.DMA((nch,)),
        ],
        compiler_params=pltpu.CompilerParams(
            collective_id=0,
            disable_semaphore_checks=True,
            disable_bounds_checks=True,
        ),
    )(x, gamma.reshape(1, n))
```

```python
import jax
import jax.numpy as jnp
from jax import lax
from jax.experimental import pallas as pl
from jax.experimental.pallas import tpu as pltpu

N_DEV = 4
EPS = 1e-5
LANES = 128
SUBLANES = 8

CHUNKS = (256, 128, 128, 128, 64, 64)
N_FAST = 4
FAR_LAG_ROWS = 330
PEERS = (2, 1, 3)
SLOT = {1: 1, 3: 2, 2: 3}


def _compiler_params():
    try:
        return pltpu.CompilerParams(
            collective_id=0,
            disable_semaphore_checks=True,
            disable_bounds_checks=True,
        )
    except TypeError:
        return pltpu.CompilerParams(collective_id=0)


def pallas_dist_rmsnorm_colshard_i_m768_n512_kernel(
    x: jax.Array,
    gamma: jax.Array,
):
    m, n = x.shape
    chunks = CHUNKS
    assert sum(chunks) == m and n % LANES == 0
    nch = len(chunks)
    offs = [sum(chunks[:c]) for c in range(nch)]
    mrows = [-(-r // LANES) for r in chunks]
    moffs = [sum(mrows[:c]) for c in range(nch)]
    mtot = sum(mrows)
    fast = [c >= nch - N_FAST for c in range(nch)]
    inv_n = 1.0 / (n * N_DEV)
    groups_per_row = LANES // SUBLANES
    steps = sorted(
        [(offs[c] + chunks[c], "near", c) for c in range(nch) if fast[c]]
        + [(offs[c] + chunks[c] + FAR_LAG_ROWS, "out", c) for c in range(nch)]
    )

    def groups(c):
        for g in range(chunks[c] // SUBLANES):
            yield (
                moffs[c] + g // groups_per_row,
                SUBLANES * (g % groups_per_row),
                offs[c] + SUBLANES * g,
            )

    def body(x_hbm, g_hbm, o_ref, xbuf, gbuf, comm, sbuf, part,
             in_sems, g_sem, send_sems, recv_sems, fast_sems):
        me = lax.axis_index("i")

        loads = [
            pltpu.make_async_copy(
                x_hbm.at[pl.ds(offs[c], chunks[c])],
                xbuf.at[pl.ds(offs[c], chunks[c])],
                in_sems.at[c],
            )
            for c in range(nch)
        ]
        for cp in loads:
            cp.start()
        g_load = pltpu.make_async_copy(g_hbm, gbuf, g_sem)
        g_load.start()

        barrier = pltpu.get_barrier_semaphore()
        for d in PEERS:
            pl.semaphore_signal(
                barrier, inc=1, device_id=((me + d) % N_DEV,),
                device_id_type=pl.DeviceIdType.MESH,
            )

        lane = lax.broadcasted_iota(jnp.int32, (SUBLANES, LANES), 1)
        sub = lax.broadcasted_iota(jnp.int32, (SUBLANES, LANES), 0)
        diag = lane - sub

        def to_column(row, b):
            wide = jnp.broadcast_to(row, (SUBLANES, LANES))
            return jnp.sum(jnp.where(diag == b, wide, 0.0), axis=1, keepdims=True)

        sends = []
        fast_copies = {}
        for c in range(nch):
            loads[c].wait()
            xv = xbuf[pl.ds(offs[c], chunks[c]), :]
            xx = xv * xv
            cols = [xx[:, LANES * k:LANES * (k + 1)] for k in range(n // LANES)]
            while len(cols) > 1:
                nxt = [cols[i] + cols[i + 1] for i in range(0, len(cols) - 1, 2)]
                if len(cols) % 2:
                    nxt.append(cols[-1])
                cols = nxt
            ssq = jnp.sum(cols[0], axis=1, keepdims=True)
            acc = {q: jnp.zeros((SUBLANES, LANES), jnp.float32)
                   for q in range(moffs[c], moffs[c] + mrows[c])}
            for q, b, r0 in groups(c):
                r = r0 - offs[c]
                acc[q] = jnp.where(diag == b, ssq[r:r + SUBLANES, :], acc[q])
            for q, a in acc.items():
                comm[0, q] = jnp.sum(a, axis=0, keepdims=True)

            if c == 0:
                pl.semaphore_wait(barrier, N_DEV - 1)

            msg = pl.ds(moffs[c], mrows[c])
            for d in PEERS:
                to_smem = fast[c] and d == 2
                cp = pltpu.make_async_remote_copy(
                    src_ref=comm.at[0, msg],
                    dst_ref=sbuf.at[msg] if to_smem else comm.at[SLOT[d], msg],
                    send_sem=send_sems.at[len(sends)],
                    recv_sem=(fast_sems.at[len(fast_copies)] if to_smem
                              else recv_sems.at[c]),
                    device_id=((me + d) % N_DEV,),
                    device_id_type=pl.DeviceIdType.MESH,
                )
                cp.start()
                sends.append(cp)
                if to_smem:
                    fast_copies[c] = cp

        g_load.wait()
        xbuf[...] = xbuf[...] * gbuf[...]
        for cp in sends:
            cp.wait_send()

        for _, kind, c in steps:
            msg_rows = range(moffs[c], moffs[c] + mrows[c])
            if kind == "near":
                got = comm.at[pl.ds(1, 2), pl.ds(moffs[c], mrows[c])]
                pltpu.make_async_copy(got, got, recv_sems.at[c]).wait()
                near = {q: (comm[0, q] + comm[1, q] + comm[2, q]) * inv_n + EPS
                        for q in msg_rows}
                for q, b, r0 in groups(c):
                    part[pl.ds(r0, SUBLANES), :] = jnp.broadcast_to(
                        to_column(near[q], b), (SUBLANES, LANES))
            elif fast[c]:
                fast_copies[c].wait_recv()
                for q, b, r0 in groups(c):
                    far = jnp.full((SUBLANES, LANES), sbuf[q, 0, b], jnp.float32)
                    for s in range(1, SUBLANES):
                        far = jnp.where(sub == s, sbuf[q, 0, b + s], far)
                    rows = pl.ds(r0, SUBLANES)
                    scale = lax.rsqrt(far * inv_n + part[rows, :])
                    for k in range(n // LANES):
                        cs = pl.ds(LANES * k, LANES)
                        o_ref[rows, cs] = xbuf[rows, cs] * scale
            else:
                got = comm.at[pl.ds(1, N_DEV - 1), pl.ds(moffs[c], mrows[c])]
                pltpu.make_async_copy(got, got, recv_sems.at[c]).wait()
                scale = {}
                for q in msg_rows:
                    tot = (comm[0, q] + comm[1, q]) + (comm[2, q] + comm[3, q])
                    scale[q] = lax.rsqrt(tot * inv_n + EPS)
                for q, b, r0 in groups(c):
                    rows = pl.ds(r0, SUBLANES)
                    o_ref[rows, :] = xbuf[rows, :] * to_column(scale[q], b)

    return pl.pallas_call(
        body,
        out_shape=jax.ShapeDtypeStruct((m, n), x.dtype),
        in_specs=[
            pl.BlockSpec(memory_space=pl.ANY),
            pl.BlockSpec(memory_space=pl.ANY),
        ],
        out_specs=pl.BlockSpec(memory_space=pltpu.VMEM),
        scratch_shapes=[
            pltpu.VMEM((m, n), jnp.float32),
            pltpu.VMEM((1, n), jnp.float32),
            pltpu.VMEM((N_DEV, mtot, 1, LANES), jnp.float32),
            pltpu.SMEM((mtot, 1, LANES), jnp.float32),
            pltpu.VMEM((m, LANES), jnp.float32),
            pltpu.SemaphoreType.DMA((nch,)),
            pltpu.SemaphoreType.DMA,
            pltpu.SemaphoreType.DMA((nch * len(PEERS),)),
            pltpu.SemaphoreType.DMA((nch,)),
            pltpu.SemaphoreType.DMA((N_FAST,)),
        ],
        compiler_params=_compiler_params(),
    )(x, gamma.reshape(1, n))
```
